```python
import numpy as np

kernel_name = "dist_sparse_attn_strided_qseq_b1_sq1024_skv1024_hq8_dh128"

def setup_inputs():
    x = np.random.randn(1, 4096, 1024).astype(np.float32)
    Wq = np.random.randn(1024, 4096).astype(np.float32) * 0.02
    K_ext = np.random.randn(1, 1024, 32, 128).astype(np.float32)
    V_ext = np.random.randn(1, 1024, 32, 128).astype(np.float32)
    Wo = np.random.randn(4096, 1024).astype(np.float32) * 0.02
    return {"x": x, "Wq": Wq, "K_ext": K_ext, "V_ext": V_ext, "Wo": Wo}

def reference(x, Wq, K_ext, V_ext, Wo):
    B, Sq, Skv, Hq, Dh = 1, 4096, 1024, 32, 128
    Q = (x @ Wq).reshape(B, Sq, Hq, Dh)
    qb = (np.arange(Sq) // 64)[:, None]
    kb = (np.arange(Skv) // 64)[None, :]
    mask = (qb == kb) | ((kb % 4) == (qb % 4))
    scores = np.einsum('bihd,bjhd->bhij', Q, K_ext).astype(np.float32) * 0.08838834764831843
    scores = np.where(mask[None, None, :, :], scores, -1e9)
    scores_max = scores.max(axis=-1, keepdims=True)
    w = np.exp(scores - scores_max)
    row_keep = mask.any(axis=1)
    w_sum = np.where(row_keep[None, None, :, None], w.sum(axis=-1, keepdims=True), 1.0)
    w = w / w_sum
    w = np.where(row_keep[None, None, :, None], w, 0.0)
    ctx = np.einsum('bhij,bjhd->bihd', w, V_ext).reshape(B, Sq, Hq * Dh)
    return ctx @ Wo
```

```python
import contextlib

import jax
import jax.numpy as jnp
from jax import lax
from jax.experimental import pallas as pl
from jax.experimental.pallas import tpu as pltpu

F32 = jnp.float32
BF16 = jnp.bfloat16

Q_SCALE = 0.08838834764831843 * 1.4426950408889634

LHS_SLOT = (4, 5, 0, 3, 6, 7, 8)
RHS_SLOT = (4, 0, 8, 7, 3, 6, 5)
X_BLK, WQ_BLK, WO_BLK = 0, 8, 16

OWN, REM = 0, 1
TRACE = False
ISSUE = ((0, 1), (2,), (3,), (4,), (5, 6), (7,), (8,), (9,), (10,))
EARLY = 2
HOLD = (0, 0, 0, 0, 1, 1, 1, 1)
SEND_AT = 4


def _scope(name):
    return jax.named_scope('z_' + name) if TRACE else contextlib.nullcontext()


def _tiles(s, rs, g, js):
    return [(s, r, g, j) for r in rs for j in js]


ALL = (0, 1, 2, 3)
_MIX_A = _tiles(REM, (0, 1), REM, (2,)) + _tiles(REM, (2,), REM, (0, 1))
_MIX_B = _tiles(REM, (0, 1), REM, (3,)) + _tiles(REM, (2,), REM, (2, 3))

SCHEDULE = (
    ((("kv", OWN, 0), ("load_kv", OWN, 2)),
     _tiles(OWN, ALL, REM, (0,)), _tiles(OWN, ALL, OWN, (0,)), None, ("x", 0)),
    ((("kv", OWN, 1), ("load_kv", OWN, 3)),
     _tiles(REM, (0,), OWN, ALL), _tiles(OWN, ALL, OWN, (1,)), None, ("wo_own", 0)),
    ((("kv", OWN, 2), ("load_wo", 1)), (), _tiles(OWN, ALL, OWN, (2,)), None, None),
    ((("kv", OWN, 3), ("load_kv", REM, 0)),
     _tiles(OWN, ALL, REM, (1,)), _tiles(OWN, ALL, OWN, (3,)), None, ("wq", 1)),
    ((("load_kv", REM, 1),),
     _tiles(REM, (1,), OWN, ALL), _tiles(REM, (0,), OWN, ALL), None, ("x", 1)),
    ((("load_kv", REM, 2), ("load_wo", 2)),
     _tiles(REM, (0, 1), REM, (0, 1)), _tiles(REM, (1,), OWN, ALL), None, ("wo_own", 1)),
    ((("kv", REM, 0), ("kv", REM, 1), ("load_kv", REM, 3)),
     _tiles(OWN, ALL, REM, (2,)), _tiles(REM, (0, 1), REM, (0, 1)), None, ("wq", 2)),
    ((("load_wo", 3),), _tiles(REM, (2,), OWN, ALL), _tiles(OWN, ALL, REM, (0,)), None, ("x", 2)),
    ((), _MIX_A, _tiles(REM, (2,), OWN, ALL), None, ("wo_own", 2)),
    ((("kv", REM, 2), ("kv", REM, 3)), _MIX_B, _MIX_A, None, ("wq", 3)),
    ((), _tiles(REM, (3,), OWN, ALL), _MIX_B, None, ("x", 3)),
    ((), _tiles(REM, (3,), REM, ALL), _tiles(REM, (3,), OWN, ALL), None, ("wo_own", 3)),
    ((("wo", 0),), (), (), (REM, 0, 0, 2), None),
    ((), (), _tiles(REM, (3,), REM, ALL), None, None),
    ((), (), _tiles(OWN, ALL, REM, (1,)), (REM, 2, 0, 2), None),
    ((("wo", 1),), (), _tiles(OWN, ALL, REM, (2,)), (REM, 0, 1, 2), None),
    ((), _tiles(OWN, ALL, REM, (3,)), (), None, None),
    ((), (), _tiles(OWN, ALL, REM, (3,)), (REM, 2, 1, 2), None),
    ((("wo", 2),), (), (), (REM, 0, 2, 4), None),
    ((), (), (), (OWN, 0, 0, 4), None),
    ((("wo", 3),), (), (), (REM, 0, 3, 4), None),
    ((), (), (), (OWN, 0, 1, 4), None),
    ((), (), (), (OWN, 0, 2, 4), None),
)


def _kind(step):
    _, qp, at, op, prep = step
    return (len(qp), len(at), op[0] if op else -1, op[3] if op else 0,
            0 if not prep else 2 if prep[0] == "wo_own" else 1)


def _pack(tiles):
    word = 0
    for a, (s, r, g, j) in enumerate(tiles):
        word |= (((4 * s + r) << 3) | (4 * g + j)) << (6 * a)
    return word


def _step_words(step, kinds):
    events, qp, at, op, prep = step
    misc = kinds.index(_kind(step)) | (bool(events) << 4)
    if op:
        misc |= (op[1] << 5) | (op[2] << 7)
    if prep:
        misc |= ({"x": X_BLK, "wq": WQ_BLK}.get(prep[0], WO_BLK) << 9) | (prep[1] << 14)
    return _pack(qp), _pack(at), misc


def _aligned(i, n):
    return i if isinstance(i, int) else pl.multiple_of(i, n)


def _quadrant_sums(q11, q12, q21, q22):
    return (q11 + q22, q21 + q22, q11 + q12, q21 - q11, q12 - q22)


class _Strassen:
    ORDER = (1, 2, 3, 4, 0, 5, 6)

    def __init__(self, product, emit):
        self.product, self.emit, self.m = product, emit, {}

    def run(self, ts):
        for t in ts:
            m = self.m
            m[t] = self.product(t)
            done = lambda *need: t in need and all(k in m for k in need)
            if done(2, 4):
                self.emit(0, 1, m[2] + m[4])
            if done(1, 3):
                self.emit(1, 0, m[1] + m[3])
            if done(0, 3, 4, 6):
                self.emit(0, 0, m[0] + m[3] - m[4] + m[6])
            if done(0, 1, 2, 5):
                self.emit(1, 1, m[0] - m[1] + m[2] + m[5])


def _body(x_hbm, wq_hbm, k_hbm, v_hbm, wo_hbm, out,
          xf, wqf, wof, kf, vf, raw, sums, qs, ctx, part_out, part_in, table,
          x_sem, wq_sem, wo_sem, kv_sem, blk_send, blk_recv, part_send, part_recv):
    me = lax.axis_index("i")
    row_peer = me ^ 1
    head_peer = 3 - me

    barrier = pltpu.get_barrier_semaphore()
    for peer in (row_peer, head_peer):
        pl.semaphore_signal(barrier, inc=1, device_id=(peer,), device_id_type=pl.DeviceIdType.MESH)

    def x_load(r):
        return pltpu.make_async_copy(x_hbm.at[:, r], xf.at[r], x_sem.at[r])

    def wq_load(j):
        return pltpu.make_async_copy(wq_hbm.at[:, pl.ds(256 * j, 256)], wqf.at[j], wq_sem.at[j])

    def wo_load(n):
        return pltpu.make_async_copy(wo_hbm.at[:, pl.ds(_aligned(256 * n, 256), 256)], wof.at[n], wo_sem.at[n])

    def kv_loads(g, j):
        first = 8 * (me if g == OWN else head_peer) + 2 * j
        return [pltpu.make_async_copy(src.at[:, :, :, first + e, :], dst.at[8 * g + 2 * j + e],
                                      kv_sem.at[4 * g + j])
                for e in range(2) for src, dst in ((k_hbm, kf), (v_hbm, vf))]

    def block_copy(base, c, peer):
        sem = (base >> 1) + c
        return pltpu.make_async_remote_copy(
            raw.at[base + c], raw.at[base + 4 + c],
            blk_send.at[sem], blk_recv.at[sem],
            device_id=(peer,), device_id_type=pl.DeviceIdType.MESH)

    def part_copy(r, n):
        return pltpu.make_async_remote_copy(
            part_out.at[4 * n + r], part_in.at[4 * n + r],
            part_send.at[4 * n + r], part_recv.at[4 * n + r],
            device_id=(row_peer,), device_id_type=pl.DeviceIdType.MESH)

    def put_block(b, quad, store_raw=True):
        for i in range(8):
            rows = pl.ds(64 * i, 64)
            quads = [quad(a, c, i) for a in range(2) for c in range(2)]
            if store_raw:
                for k, q in enumerate(quads):
                    raw[b, k, rows, :] = q.astype(BF16)
            for k, q in enumerate(_quadrant_sums(*quads)):
                sums[b, k, rows, :] = q.astype(BF16)

    def prep_own_x(r):
        put_block(X_BLK + r, lambda a, b, i: xf[r, 2 * a + i % 2, :, pl.ds(512 * b + 128 * (i // 2), 128)])

    def prep_own_wq(j):
        put_block(WQ_BLK + j,
                  lambda a, b, i: wqf[j, pl.ds(512 * a + 64 * i, 64), pl.ds(128 * b, 128)] * Q_SCALE)

    def prep_own_wo(n):
        put_block(WO_BLK + n, lambda a, b, i: wof[
            n, pl.ds(128 * (2 * (i // 2) + a) + 64 * (i % 2), 64), pl.ds(128 * b, 128)])

    def prep_received(blk):
        put_block(blk, lambda a, b, i: raw[blk, 2 * a + b, pl.ds(64 * i, 64), :].astype(F32),
                  store_raw=False)

    def operand(blk, slot, rows=slice(None)):
        return raw[blk, slot, rows, :] if slot < 4 else sums[blk, slot - 4, rows, :]

    def q_projection(sr, gj):
        xb, wb, tile = X_BLK + sr, WQ_BLK + gj, sr * 8 + gj

        def product(t):
            lhs = jnp.concatenate(
                [operand(xb, LHS_SLOT[t], pl.ds(128 * k, 128)) for k in range(4)], axis=1)
            return jnp.dot(lhs, operand(wb, RHS_SLOT[t]), preferred_element_type=F32)

        def emit(a, b, val):
            qs[2 * tile + b, 128 * a:128 * (a + 1), :] = val.astype(BF16)

        return _Strassen(product, emit)

    class Attention:
        def __init__(self, sr, gj):
            self.r, self.sr, self.gj = sr & 3, sr, gj
            self.p = {}

        def scores(self):
            for e in range(2):
                k = kf[2 * self.gj + e, :, self.r].reshape(256, 128).astype(BF16)
                q = qs[2 * (self.sr * 8 + self.gj) + e]
                s = lax.dot_general(q, k, (((1,), (1,)), ((), ())), preferred_element_type=F32)
                p = jnp.exp2(s - jnp.max(s, axis=-1, keepdims=True))
                self.p[e] = (p.astype(BF16), jnp.sum(p, axis=-1, keepdims=True))

        def values(self):
            o = []
            for e in range(2):
                p, l = self.p[e]
                v = vf[2 * self.gj + e, :, self.r].reshape(256, 128).astype(BF16)
                inv = pl.reciprocal(l, approx=True)
                inv = inv * (2.0 - l * inv)
                o.append(jnp.dot(p, v, preferred_element_type=F32) * inv)
            quads = (o[0][:128], o[1][:128], o[0][128:], o[1][128:])
            slots = quads + _quadrant_sums(*quads)
            for t in range(7):
                ctx[self.sr, t, self.gj] = slots[LHS_SLOT[t]].astype(BF16)

    def out_projection(s, rs, n):
        def product(t):
            lhs = jnp.concatenate(
                [jnp.concatenate([ctx[4 * s + r, t, k] for k in range(8)], axis=1) for r in rs], axis=0)
            rhs = jnp.concatenate([operand(WO_BLK + 4 * g + n, RHS_SLOT[t]) for g in range(2)], axis=0)
            return jnp.dot(lhs, rhs, preferred_element_type=F32)

        def emit(a, b, vals):
            for i, r in enumerate(rs):
                val = vals[128 * i:128 * (i + 1)]
                if s == REM:
                    part_out[4 * n + r, b, 128 * a:128 * (a + 1), :] = val.astype(BF16)
                else:
                    val = val + part_in[4 * n + r, b, 128 * a:128 * (a + 1), :].astype(F32)
                    for j in range(2):
                        rows = pl.ds(_aligned(256 * (2 * a + j) + 64 * r, 64), 64)
                        cols = pl.ds(_aligned(256 * n + 128 * b, 128), 128)
                        out[0, rows, cols] = val[64 * j:64 * (j + 1)].astype(BF16)

        return _Strassen(product, emit)

    queue = [[f(c)] for c in range(4) for f in (wq_load, x_load)] + [kv_loads(OWN, 0), [wo_load(0)], kv_loads(OWN, 1)]

    def issue(k):
        if k < len(queue):
            for cp in queue[k]:
                cp.start()

    def run_event(ev):
        if ev[0] == "kv":
            for cp in kv_loads(ev[1], ev[2]):
                cp.wait()
        elif ev[0] == "load_kv":
            for cp in kv_loads(ev[1], ev[2]):
                cp.start()
        elif ev[0] == "load_wo":
            wo_load(ev[1]).start()
        else:
            base = {"x": X_BLK, "wq": WQ_BLK, "wo": WO_BLK}[ev[0]]
            block_copy(base, ev[1], row_peer).wait_recv()
            prep_received(base + 4 + ev[1])

    def project(tiles):
        for tile in tiles:
            q_projection(*tile).run(_Strassen.ORDER)

    for k in ISSUE[0]:
        issue(k)
    kinds = []
    for st in SCHEDULE:
        if _kind(st) not in kinds:
            kinds.append(_kind(st))
    for k, st in enumerate(SCHEDULE):
        for c, word in enumerate(_step_words(st, kinds)):
            table[3 * k + c] = jnp.int32(word)
    ready = []
    for k in range(8):
        c = k // 2
        with _scope("L%d" % k):
            (x_load(c) if k % 2 else wq_load(c)).wait()
        for nxt in ISSUE[k + 1]:
            issue(nxt)
        (prep_own_x if k % 2 else prep_own_wq)(c)
        if k == 0:
            pl.semaphore_wait(barrier, 2)
            block_copy(WQ_BLK, 0, head_peer).start()
        if k == 1:
            block_copy(X_BLK, 0, row_peer).start()
        ready += [(c, j) for j in range(c + 1)] if k % 2 else [(r, c) for r in range(c)]
        keep = HOLD[k]
        project(ready[:len(ready) - keep])
        ready = ready[len(ready) - keep:]
        if k == SEND_AT:
            for c in range(1, k // 2 + 1):
                block_copy(WQ_BLK, c, head_peer).start()
            for c in range(1, (k + 1) // 2):
                block_copy(X_BLK, c, row_peer).start()
    for c in range(SEND_AT // 2 + 1, 4):
        block_copy(WQ_BLK, c, head_peer).start()
    for c in range((SEND_AT + 1) // 2, 4):
        block_copy(X_BLK, c, row_peer).start()
    with _scope("L8"):
        block_copy(WQ_BLK, 0, head_peer).wait_recv()
    prep_received(WQ_BLK + 4)
    project(ready)

    def run_step(i, kind):
        n_qp, n_at, op_shard, n_op, prep = kind
        unpack = lambda word, n: [((word >> (6 * a + 3)) & 7, (word >> (6 * a)) & 7) for a in range(n)]
        qp = unpack(table[3 * i], n_qp)
        att = [Attention(*tile) for tile in unpack(table[3 * i + 1], n_at)]
        misc = table[3 * i + 2]
        if op_shard >= 0:
            r0, n = (misc >> 5) & 2, (misc >> 7) & 3
            rs = (r0, r0 + 1) if n_op == 2 else ALL
            mm = out_projection(op_shard, rs, n)

            def first():
                if op_shard == OWN:
                    for r in rs:
                        part_copy(r, n).wait_recv()
                mm.run(_Strassen.ORDER[:4])

            def second():
                mm.run(_Strassen.ORDER[4:])
                if op_shard == REM:
                    for r in rs:
                        part_copy(r, n).start()
        else:
            first = lambda: project(qp[:2])
            second = lambda: project(qp[2:])

        base, c = (misc >> 9) & 24, (misc >> 14) & 3
        if prep == 1:
            block_copy(base, c, row_peer).wait_recv()
        elif prep == 2:
            wo_load(c).wait()

        def prepare():
            if prep == 1:
                prep_received(base + 4 + c)
            elif prep == 2:
                prep_own_wo(c)

        if not att:
            first()
            prepare()
            second()
        elif not qp and op_shard < 0:
            att[0].scores()
            for a in range(len(att)):
                if a + 1 < len(att):
                    att[a + 1].scores()
                if a + 2 == len(att):
                    prepare()
                att[a].values()
        else:
            att[0].scores()
            att[1].scores()
            if EARLY == 2:
                prepare()
            first()
            att[0].values()
            att[1].values()
            att[2].scores()
            att[3].scores()
            if EARLY == 1:
                prepare()
            second()
            if not EARLY:
                prepare()
            att[2].values()
            att[3].values()
        if prep == 2:
            block_copy(WO_BLK, c, head_peer).start()

    def step(i, carry):
        misc = table[3 * i + 2]

        @pl.when((misc & 16) != 0)
        def _():
            for k, st in enumerate(SCHEDULE):
                if st[0]:
                    @pl.when(i == k)
                    def _(st=st):
                        for ev in st[0]:
                            run_event(ev)

        def branch(kind):
            def run():
                with _scope("S%d%d%d%d%d" % (kind[0], kind[1], kind[2] + 1, kind[3], kind[4])):
                    run_step(i, kind)
            return run

        lax.switch(misc & 15, [branch(kind) for kind in kinds])
        return carry

    lax.fori_loop(0, len(SCHEDULE), step, None)

    last_rs, last_n, pending = ALL, 3, []
    mm = out_projection(OWN, last_rs, last_n)
    finish, mm.emit = mm.emit, lambda *quadrant: pending.append(quadrant)
    with _scope("T0"):
        mm.run(_Strassen.ORDER)
    with _scope("T1"):
        for r in last_rs:
            part_copy(r, last_n).wait_recv()
    for quadrant in pending:
        finish(*quadrant)

    for base in (X_BLK, WQ_BLK, WO_BLK):
        for c in range(4):
            block_copy(base, c, row_peer).wait_send()
    for n in range(4):
        for r in range(4):
            part_copy(r, n).wait_send()


def pallas_dist_sparse_attn_strided_qseq_b1_sq1024_skv1024_hq8_dh128_kernel(
    x: jax.Array,
    Wq: jax.Array,
    K_ext: jax.Array,
    V_ext: jax.Array,
    Wo: jax.Array,
):
    dma = pltpu.SemaphoreType.DMA
    return pl.pallas_call(
        _body,
        out_shape=pltpu.VMEM((1, 1024, 1024), BF16),
        in_specs=[pl.BlockSpec(memory_space=pl.ANY)] * 5,
        out_specs=pl.BlockSpec(memory_space=pltpu.VMEM),
        scratch_shapes=[
            pltpu.VMEM((4, 4, 64, 1024), F32),
            pltpu.VMEM((4, 1024, 256), F32),
            pltpu.VMEM((4, 1024, 256), F32),
            pltpu.VMEM((16, 4, 4, 64, 128), F32),
            pltpu.VMEM((16, 4, 4, 64, 128), F32),
            pltpu.VMEM((24, 4, 512, 128), BF16),
            pltpu.VMEM((24, 5, 512, 128), BF16),
            pltpu.VMEM((128, 256, 128), BF16),
            pltpu.VMEM((8, 7, 8, 128, 128), BF16),
            pltpu.VMEM((16, 2, 256, 128), BF16),
            pltpu.VMEM((16, 2, 256, 128), BF16),
            pltpu.SMEM((3 * len(SCHEDULE),), jnp.int32),
            dma((4,)), dma((4,)), dma((4,)), dma((8,)),
            dma((12,)), dma((12,)), dma((16,)), dma((16,)),
        ],
        compiler_params=pltpu.CompilerParams(collective_id=0, vmem_limit_bytes=100 * 1024 * 1024),
    )(
        x.reshape(4, 4, 64, 1024),
        Wq,
        K_ext.reshape(4, 4, 64, 32, 128),
        V_ext.reshape(4, 4, 64, 32, 128),
        Wo,
    )
```

```python
import functools

import jax
import jax.numpy as jnp
from jax import lax
from jax.experimental import pallas as pl
from jax.experimental.pallas import tpu as pltpu

F32 = jnp.float32
BF16 = jnp.bfloat16

Q_SCALE = 0.08838834764831843 * 1.4426950408889634

LHS_SLOT = (4, 5, 0, 3, 6, 7, 8)
RHS_SLOT = (4, 0, 8, 7, 3, 6, 5)
X_BLK, WQ_BLK, WO_BLK = 0, 8, 16

OWN, REM = 0, 1

EARLY_PARTS = 2
LOOKAHEAD = 2


def _tiles(s, rs, g, js):
    return [(s, r, g, j) for r in rs for j in js]


ALL = (0, 1, 2, 3)
_MIX_A = _tiles(REM, (0, 1), REM, (2,)) + _tiles(REM, (2,), REM, (0, 1))
_MIX_B = _tiles(REM, (0, 1), REM, (3,)) + _tiles(REM, (2,), REM, (2, 3))

def _own(kind, *residues):
    return _tiles(kind, residues, OWN, ALL)


class _Step:
    def __init__(self, q=(), att=(), out=None, prep=None,
                 wait_kv=None, load_kv=None, load_wo=None, early=None):
        self.q, self.att, self.out, self.prep = q, att, out, prep
        self.wait_kv, self.load_kv, self.load_wo, self.early = wait_kv, load_kv, load_wo, early
        self.kind = (len(q), len(att), out[0] if out else -1, out[3] if out else 0,
                     prep[0] == "wo_own" if prep else None)

    def words(self, kinds):
        def pack(tiles):
            return sum((((4 * s + r) << 3) | (4 * g + j)) << (6 * a) for a, (s, r, g, j) in enumerate(tiles))

        def block(what, c):
            return {"x": X_BLK, "wq": WQ_BLK}.get(what, WO_BLK) | c

        misc, moves = kinds.index(self.kind), 0
        if self.out:
            misc |= (self.out[1] << 4) | (self.out[2] << 6)
        if self.prep:
            misc |= block(*self.prep) << 8
        if self.wait_kv:
            moves |= 8 | (4 * self.wait_kv[0] + self.wait_kv[1])
        if self.load_kv:
            moves |= (8 | (4 * self.load_kv[0] + self.load_kv[1])) << 4
        if self.load_wo is not None:
            moves |= (4 | self.load_wo) << 8
        if self.early:
            moves |= ((64 if self.early[0] == "wo_own" else 32) | block(*self.early)) << 12
        return pack(self.q), pack(self.att), misc, moves


SCHEDULE = (
    _Step(att=_own(OWN, 0), wait_kv=(OWN, 0), load_kv=(OWN, 2)),
    _Step(q=_tiles(OWN, ALL, REM, (0,)), early=("wq", 0)),
    _Step(q=_own(REM, 0), att=_own(OWN, 1), prep=("x", 0), wait_kv=(OWN, 1), load_kv=(OWN, 3)),
    _Step(att=_own(OWN, 2), wait_kv=(OWN, 2), load_kv=(REM, 0)),
    _Step(att=_own(OWN, 3), wait_kv=(OWN, 3), load_kv=(REM, 1)),
    _Step(q=_own(REM, 1), att=_own(REM, 0), prep=("x", 1), wait_kv=(REM, 0), load_wo=0),
    _Step(q=_tiles(REM, (0, 1), REM, (0, 1)), att=_own(REM, 1), prep=("wq", 1),
          wait_kv=(REM, 1), load_kv=(REM, 2)),
    _Step(q=_tiles(OWN, ALL, REM, (1,)), att=_tiles(REM, (0, 1), REM, (0, 1)), prep=("wo_own", 0),
          wait_kv=(REM, 2), load_kv=(REM, 3)),
    _Step(q=_own(REM, 2), att=_tiles(OWN, ALL, REM, (0,)), prep=("x", 2), wait_kv=(REM, 3), load_wo=1),
    _Step(q=_MIX_A, att=_own(REM, 2), prep=("wq", 2), load_wo=2),
    _Step(q=_MIX_B, att=_MIX_A, prep=("wq", 3), load_wo=3, early=("wo_own", 1)),
    _Step(q=_own(REM, 3), att=_MIX_B, prep=("x", 3)),
    _Step(q=_tiles(REM, (3,), REM, ALL), att=_own(REM, 3), prep=("wo_own", 2)),
    _Step(att=_tiles(REM, (3,), REM, ALL), out=(REM, 0, 0, 2), early=("wo", 0)),
    _Step(out=(REM, 2, 0, 2)),
    _Step(q=_tiles(OWN, ALL, REM, (2,)), att=_tiles(OWN, ALL, REM, (1,)), prep=("wo_own", 3)),
    _Step(out=(REM, 0, 1, 4), early=("wo", 1)),
    _Step(q=_tiles(OWN, ALL, REM, (3,)), att=_tiles(OWN, ALL, REM, (2,))),
    _Step(att=_tiles(OWN, ALL, REM, (3,))),
    _Step(out=(REM, 0, 2, 4), early=("wo", 2)),
    _Step(out=(OWN, 0, 0, 4)),
    _Step(out=(OWN, 0, 1, 2)),
    _Step(out=(REM, 0, 3, 2), early=("wo", 3)),
    _Step(out=(REM, 2, 3, 2)),
    _Step(out=(OWN, 2, 1, 2)),
    _Step(out=(OWN, 0, 2, 4)),
)
WORDS = 4


def _aligned(i, n):
    return i if isinstance(i, int) else pl.multiple_of(i, n)


def _quadrant_sums(q11, q12, q21, q22):
    return (q11 + q22, q21 + q22, q11 + q12, q21 - q11, q12 - q22)


class _Strassen:
    ORDER = (1, 2, 3, 4, 0, 5, 6)

    def __init__(self, product, emit):
        self.product, self.emit, self.m = product, emit, {}

    def run(self, ts):
        for t in ts:
            m = self.m
            m[t] = self.product(t)
            done = lambda *need: t in need and all(k in m for k in need)
            if done(2, 4):
                self.emit(0, 1, m[2] + m[4])
            if done(1, 3):
                self.emit(1, 0, m[1] + m[3])
            if done(0, 3, 4, 6):
                self.emit(0, 0, m[0] + m[3] - m[4] + m[6])
            if done(0, 1, 2, 5):
                self.emit(1, 1, m[0] - m[1] + m[2] + m[5])


def _body(x_hbm, wq_hbm, k_hbm, v_hbm, wo_hbm, out,
          xf, wqf, wof, kvf, raw, sums, q_acc, qs, ctx, part_out, part_in, table,
          x_sem, wq_sem, wo_sem, kv_sem, blk_send, blk_recv, part_send, part_recv):
    me = lax.axis_index("i")
    row_peer = me ^ 1
    head_peer = 3 - me

    barrier = pltpu.get_barrier_semaphore()
    for peer in (row_peer, head_peer):
        pl.semaphore_signal(barrier, inc=1, device_id=(peer,), device_id_type=pl.DeviceIdType.MESH)

    def quarter_loads(q):
        k = pl.ds(_aligned(256 * q, 256), 256)
        return [pltpu.make_async_copy(wq_hbm.at[k], wqf.at[q], wq_sem.at[q]),
                pltpu.make_async_copy(x_hbm.at[:, :, :, k], xf.at[q], x_sem.at[q])]

    def wo_load(n):
        return pltpu.make_async_copy(wo_hbm.at[:, pl.ds(_aligned(256 * n, 256), 256)], wof.at[n], wo_sem.at[n])

    def start_kv(group):
        first, r = 8 * jnp.where(group < 4, me, head_peer), group & 3
        for e, src in enumerate((k_hbm, v_hbm)):
            for h in range(8):
                pltpu.make_async_copy(src.at[:, r, :, first + h, :], kvf.at[group, e, h],
                                      kv_sem.at[group]).start()

    def block_copy(base, c, peer, part=()):
        sem = (base >> 1) + c
        return pltpu.make_async_remote_copy(
            raw.at[(base + c,) + part], raw.at[(base + 4 + c,) + part],
            blk_send.at[base >> 3], blk_recv.at[sem],
            device_id=(peer,), device_id_type=pl.DeviceIdType.MESH)

    def part_copy(r, n):
        return pltpu.make_async_remote_copy(
            part_out.at[4 * n + r], part_in.at[4 * n + r],
            part_send, part_recv.at[4 * n + r],
            device_id=(row_peer,), device_id_type=pl.DeviceIdType.MESH)

    def put_tile(blk, k, quad, store_raw=True):
        for h in range(2):
            rows = pl.ds(64 * h, 64)
            quads = [quad(a, b, h) for a in range(2) for b in range(2)]
            if store_raw:
                for i, q in enumerate(quads):
                    raw[blk, k, i, rows, :] = q.astype(BF16)
            for i, q in enumerate(_quadrant_sums(*quads)):
                sums[blk, k, i, rows, :] = q.astype(BF16)

    def prep_own_x(r, k):
        put_tile(X_BLK + r, k, lambda a, b, h: xf[k, 2 * a + h, r, :, pl.ds(128 * b, 128)])

    def prep_own_wq(j, k):
        put_tile(WQ_BLK + j, k, lambda a, b, h: wqf[
            k, pl.ds(128 * a + 64 * h, 64), pl.ds(256 * j + 128 * b, 128)] * Q_SCALE)

    def prep_own_wo(n):
        for k in range(4):
            put_tile(WO_BLK + n, k, lambda a, b, h: wof[
                n, pl.ds(256 * k + 128 * a + 64 * h, 64), pl.ds(128 * b, 128)])

    def prep_received(blk):
        for k in range(4):
            put_tile(blk, k, lambda a, b, h: raw[blk, k, 2 * a + b, pl.ds(64 * h, 64), :].astype(F32),
                     store_raw=False)

    def operand(blk, k, slot):
        return raw[blk, k, slot] if slot < 4 else sums[blk, k, slot - 4]

    def q_projection(sr, gj):
        xb, wb, tile = X_BLK + sr, WQ_BLK + gj, sr * 8 + gj

        def product(t):
            lhs = jnp.concatenate(
                [operand(xb, k, LHS_SLOT[t]) for k in range(4)], axis=1)
            rhs = jnp.concatenate([operand(wb, k, RHS_SLOT[t]) for k in range(4)], axis=0)
            return jnp.dot(lhs, rhs, preferred_element_type=F32)

        def emit(a, b, val):
            qs[2 * tile + b, 128 * a:128 * (a + 1), :] = val.astype(BF16)

        return _Strassen(product, emit)

    class Attention:
        def __init__(self, sr, gj):
            self.sr, self.gj = sr, gj
            self.p = {}

        def keys(self, which, e):
            block = kvf[(self.gj & 4) + (self.sr & 3), which, 2 * (self.gj & 3) + e]
            return block.reshape(256, 128).astype(BF16)

        def scores(self):
            for e in range(2):
                k = self.keys(0, e)
                q = qs[2 * (self.sr * 8 + self.gj) + e]
                s = lax.dot_general(q, k, (((1,), (1,)), ((), ())), preferred_element_type=F32)
                p = jnp.exp2(s - jnp.max(s, axis=-1, keepdims=True))
                self.p[e] = (p.astype(BF16), jnp.sum(p, axis=-1, keepdims=True))

        def values(self):
            o = []
            for e in range(2):
                p, l = self.p[e]
                v = self.keys(1, e)
                inv = pl.reciprocal(l, approx=True)
                inv = inv * (2.0 - l * inv)
                o.append(jnp.dot(p, v, preferred_element_type=F32) * inv)
            quads = (o[0][:128], o[1][:128], o[0][128:], o[1][128:])
            slots = quads + _quadrant_sums(*quads)
            for t in range(7):
                ctx[self.sr, t, self.gj] = slots[LHS_SLOT[t]].astype(BF16)

    def out_projection(s, rs, n, defer=None):
        def product(t):
            lhs = jnp.concatenate(
                [jnp.concatenate([ctx[4 * s + r, t, k] for k in range(8)], axis=1) for r in rs], axis=0)
            rhs = jnp.concatenate([operand(WO_BLK + 4 * g + n, k, RHS_SLOT[t])
                                   for g in range(2) for k in range(4)], axis=0)
            return jnp.dot(lhs, rhs, preferred_element_type=F32)

        def finish(r, a, b, val):
            val = val + part_in[4 * n + r, b, 128 * a:128 * (a + 1), :].astype(F32)
            for j in range(2):
                rows = pl.ds(_aligned(256 * (2 * a + j) + 64 * r, 64), 64)
                cols = pl.ds(_aligned(256 * n + 128 * b, 128), 128)
                out[0, rows, cols] = val[64 * j:64 * (j + 1)].astype(BF16)

        def emit(a, b, vals):
            for i, r in enumerate(rs):
                val = vals[128 * i:128 * (i + 1)]
                if s == REM:
                    part_out[4 * n + r, b, 128 * a:128 * (a + 1), :] = val.astype(BF16)
                elif defer and r in defer[0]:
                    defer[1].append(functools.partial(finish, r, a, b, val))
                else:
                    finish(r, a, b, val)

        return _Strassen(product, emit)

    for cp in quarter_loads(0) + quarter_loads(1)[:1]:
        cp.start()
    used = [st.kind for st in SCHEDULE]
    kinds = sorted(dict.fromkeys(used), key=used.count, reverse=True)
    for k, st in enumerate(SCHEDULE):
        for c, word in enumerate(st.words(kinds)):
            table[WORDS * k + c] = jnp.int32(word)

    def project(tiles):
        for tile in tiles:
            q_projection(*tile).run(_Strassen.ORDER)

    q_acc[...] = jnp.zeros(q_acc.shape, F32)
    pl.semaphore_wait(barrier, 2)

    def quarter(q, carry):
        wq_cp, x_cp = quarter_loads(q)
        wq_cp.wait()

        pl.when(q < 3)(lambda: quarter_loads(q + 1)[1].start())
        prep_own_wq(0, q)
        block_copy(WQ_BLK, 0, head_peer, (q,)).start()
        for j in (1, 2, 3):
            prep_own_wq(j, q)

        @pl.when(q == 0)
        def _():
            block_copy(WQ_BLK, 1, head_peer, (0, pl.ds(0, 3))).start()

        @pl.when(q == 3)
        def _():
            block_copy(WQ_BLK, 1, head_peer, (0, pl.ds(3, 1))).start()
            block_copy(WQ_BLK, 1, head_peer, (pl.ds(1, 3),)).start()
            block_copy(WQ_BLK, 2, head_peer).start()
            block_copy(WQ_BLK, 3, head_peer).start()

        x_cp.wait()

        pl.when(q < 2)(lambda: quarter_loads(q + 2)[0].start())
        pl.when(q >= 2)(lambda: start_kv(q - 2))
        prep_own_x(0, q)
        prep_own_x(1, q)
        block_copy(X_BLK, 0, row_peer, (q,)).start()

        @pl.when(q == 0)
        def _():
            block_copy(X_BLK, 1, row_peer, (0, pl.ds(0, 3))).start()

        @pl.when(q == 3)
        def _():
            block_copy(X_BLK, 1, row_peer, (0, pl.ds(3, 1))).start()
            block_copy(X_BLK, 1, row_peer, (pl.ds(1, 3),)).start()

        for r in ALL:
            if r < 2:
                prep_own_x(r + 2, q)

            def product(t):
                rhs = jnp.concatenate([operand(WQ_BLK + j, q, RHS_SLOT[t]) for j in ALL], axis=1)
                return jnp.dot(operand(X_BLK + r, q, LHS_SLOT[t]), rhs, preferred_element_type=F32)

            def emit(a, b, val):
                for j in ALL:
                    total = q_acc[r, 2 * a + b, j] + val[:, 128 * j:128 * (j + 1)]
                    q_acc[r, 2 * a + b, j] = total
                    qs[2 * (8 * r + j) + b, 128 * a:128 * (a + 1), :] = total.astype(BF16)

            _Strassen(product, emit).run(_Strassen.ORDER)
        return carry

    lax.fori_loop(0, 4, quarter, None)
    for c in (2, 3):
        block_copy(X_BLK, c, row_peer).start()

    def run_step(i, kind):
        n_qp, n_at, op_shard, n_op, own_prep = kind
        unpack = lambda word, n: [((word >> (6 * a + 3)) & 7, (word >> (6 * a)) & 7) for a in range(n)]
        qp = unpack(table[WORDS * i], n_qp)
        att = [Attention(*tile) for tile in unpack(table[WORDS * i + 1], n_at)]
        misc = table[WORDS * i + 2]
        base, c = (misc >> 8) & 24, (misc >> 8) & 3
        if own_prep:
            wo_load(c).wait()
        elif own_prep is not None:
            block_copy(base, c, row_peer).wait_recv()

        if op_shard >= 0:
            r0, n = (misc >> 4) & 2, (misc >> 6) & 3
            rs = (r0, r0 + 1) if n_op == 2 else ALL
            if op_shard == OWN:
                for r in rs:
                    part_copy(r, n).wait_recv()
            mm = out_projection(op_shard, rs, n)
            matmuls = [functools.partial(mm.run, ts) for ts in (_Strassen.ORDER[:4], _Strassen.ORDER[4:])]
        else:
            matmuls = [functools.partial(project, qp[a:a + 2]) for a in range(0, n_qp, 2)]

        if not att:
            for run in matmuls:
                run()
        elif not matmuls:
            for a in range(n_at + LOOKAHEAD):
                if a < n_at:
                    att[a].scores()
                if a >= LOOKAHEAD:
                    att[a - LOOKAHEAD].values()
        else:
            for a, run in enumerate(matmuls):
                att[2 * a].scores()
                att[2 * a + 1].scores()
                if a == 0 and own_prep:
                    prep_own_wo(c)
                elif a == 0 and own_prep is not None:
                    prep_received(base + 4 + c)
                run()
                att[2 * a].values()
                att[2 * a + 1].values()

        if own_prep:
            block_copy(WO_BLK, c, head_peer).start()
        if op_shard == REM:
            for r in rs:
                part_copy(r, n).start()

    def step(i, carry):
        moves = table[WORDS * i + 3]

        @pl.when(moves != 0)
        def _():
            @pl.when((moves & 8) != 0)
            def _():
                group = kvf.at[moves & 7]
                pltpu.make_async_copy(group, group, kv_sem.at[moves & 7]).wait()

            pl.when((moves & (8 << 4)) != 0)(lambda: start_kv((moves >> 4) & 7))
            pl.when((moves & (4 << 8)) != 0)(lambda: wo_load((moves >> 8) & 3).start())
            base, c = (moves >> 12) & 24, (moves >> 12) & 3

            @pl.when((moves & (32 << 12)) != 0)
            def _():
                block_copy(base, c, row_peer).wait_recv()
                prep_received(base + 4 + c)

            @pl.when((moves & (64 << 12)) != 0)
            def _():
                wo_load(c).wait()
                prep_own_wo(c)
                block_copy(WO_BLK, c, head_peer).start()

        lax.switch(table[WORDS * i + 2] & 15, [functools.partial(run_step, i, kind) for kind in kinds])
        return carry

    lax.fori_loop(0, len(SCHEDULE), step, None)

    for r in range(EARLY_PARTS):
        part_copy(r, 3).wait_recv()
    pending = []
    mm = out_projection(OWN, ALL, 3, defer=(range(EARLY_PARTS, 4), pending))
    mm.run(_Strassen.ORDER)
    for r in range(EARLY_PARTS, 4):
        part_copy(r, 3).wait_recv()
    for finish in pending:
        finish()

    for kind, base in enumerate((X_BLK, WQ_BLK, WO_BLK)):
        sent = raw.at[pl.ds(base, 4)]
        pltpu.make_async_copy(sent, sent, blk_send.at[kind]).wait()
    pltpu.make_async_copy(part_out, part_out, part_send).wait()


def pallas_dist_sparse_attn_strided_qseq_b1_sq1024_skv1024_hq8_dh128_kernel(
    x: jax.Array,
    Wq: jax.Array,
    K_ext: jax.Array,
    V_ext: jax.Array,
    Wo: jax.Array,
):
    dma = pltpu.SemaphoreType.DMA
    return pl.pallas_call(
        _body,
        out_shape=pltpu.VMEM((1, 1024, 1024), BF16),
        in_specs=[pl.BlockSpec(memory_space=pl.ANY)] * 5,
        out_specs=pl.BlockSpec(memory_space=pltpu.VMEM),
        scratch_shapes=[
            pltpu.VMEM((4, 4, 4, 64, 256), F32),
            pltpu.VMEM((4, 256, 1024), F32),
            pltpu.VMEM((4, 1024, 256), F32),
            pltpu.VMEM((8, 2, 8, 4, 64, 128), F32),
            pltpu.VMEM((24, 4, 4, 128, 128), BF16),
            pltpu.VMEM((24, 4, 5, 128, 128), BF16),
            pltpu.VMEM((4, 4, 4, 128, 128), F32),
            pltpu.VMEM((128, 256, 128), BF16),
            pltpu.VMEM((8, 7, 8, 128, 128), BF16),
            pltpu.VMEM((16, 2, 256, 128), BF16),
            pltpu.VMEM((16, 2, 256, 128), BF16),
            pltpu.SMEM((WORDS * len(SCHEDULE),), jnp.int32),
            dma((4,)), dma((4,)), dma((4,)), dma((8,)),
            dma((3,)), dma((12,)), dma, dma((16,)),
        ],
        compiler_params=pltpu.CompilerParams(collective_id=0, vmem_limit_bytes=100 * 1024 * 1024),
    )(
        x.reshape(4, 4, 64, 1024),
        Wq,
        K_ext.reshape(4, 4, 64, 32, 128),
        V_ext.reshape(4, 4, 64, 32, 128),
        Wo,
    )
```

```python
import functools

import jax
import jax.numpy as jnp
from jax import lax
from jax.experimental import pallas as pl
from jax.experimental.pallas import tpu as pltpu

F32 = jnp.float32
BF16 = jnp.bfloat16

Q_SCALE = 0.08838834764831843 * 1.4426950408889634

LHS_SLOT = (4, 5, 0, 3, 6, 7, 8)
RHS_SLOT = (4, 0, 8, 7, 3, 6, 5)
X_BLK, WQ_BLK, WO_BLK = 0, 8, 16

OWN, REM = 0, 1

EARLY_PARTS = 2
LOOKAHEAD = 2


def _tiles(s, rs, g, js):
    return [(s, r, g, j) for r in rs for j in js]


ALL = (0, 1, 2, 3)
_MIX_A = _tiles(REM, (0, 1), REM, (2,)) + _tiles(REM, (2,), REM, (0, 1))
_MIX_B = _tiles(REM, (0, 1), REM, (3,)) + _tiles(REM, (2,), REM, (2, 3))

def _own(kind, *residues):
    return _tiles(kind, residues, OWN, ALL)


class _Step:
    def __init__(self, q=(), att=(), out=None, prep=None,
                 wait_kv=None, load_kv=None, load_wo=None, early=None):
        self.q, self.att, self.out, self.prep = q, att, out, prep
        self.wait_kv, self.load_kv, self.load_wo, self.early = wait_kv, load_kv, load_wo, early
        self.kind = (len(q), len(att), out[0] if out else -1, out[3] if out else 0,
                     prep[0] == "wo_own" if prep else None)

    def words(self, kinds):
        def pack(tiles):
            return sum((((4 * s + r) << 3) | (4 * g + j)) << (6 * a) for a, (s, r, g, j) in enumerate(tiles))

        def block(what, c):
            return {"x": X_BLK, "wq": WQ_BLK}.get(what, WO_BLK) | c

        misc, moves = kinds.index(self.kind), 0
        if self.out:
            misc |= (self.out[1] << 4) | (self.out[2] << 6)
        if self.prep:
            misc |= block(*self.prep) << 8
        if self.wait_kv:
            moves |= 8 | (4 * self.wait_kv[0] + self.wait_kv[1])
        if self.load_kv:
            moves |= (8 | (4 * self.load_kv[0] + self.load_kv[1])) << 4
        if self.load_wo is not None:
            moves |= (4 | self.load_wo) << 8
        if self.early:
            moves |= ((64 if self.early[0] == "wo_own" else 32) | block(*self.early)) << 12
        return pack(self.q), pack(self.att), misc, moves


SCHEDULE = (
    _Step(att=_own(OWN, 0), wait_kv=(OWN, 0), load_kv=(OWN, 2)),
    _Step(q=_tiles(OWN, ALL, REM, (0,)), early=("wq", 0)),
    _Step(q=_own(REM, 0), att=_own(OWN, 1), prep=("x", 0), wait_kv=(OWN, 1), load_kv=(OWN, 3)),
    _Step(att=_own(OWN, 2), wait_kv=(OWN, 2), load_kv=(REM, 0)),
    _Step(att=_own(OWN, 3), wait_kv=(OWN, 3), load_kv=(REM, 1)),
    _Step(q=_own(REM, 1), att=_own(REM, 0), prep=("x", 1), wait_kv=(REM, 0), load_wo=0),
    _Step(q=_tiles(REM, (0, 1), REM, (0, 1)), att=_own(REM, 1), prep=("wq", 1),
          wait_kv=(REM, 1), load_kv=(REM, 2)),
    _Step(q=_tiles(OWN, ALL, REM, (1,)), att=_tiles(REM, (0, 1), REM, (0, 1)), prep=("wo_own", 0),
          wait_kv=(REM, 2), load_kv=(REM, 3)),
    _Step(q=_own(REM, 2), att=_tiles(OWN, ALL, REM, (0,)), prep=("x", 2), wait_kv=(REM, 3), load_wo=1),
    _Step(q=_MIX_A, att=_own(REM, 2), prep=("wq", 2), load_wo=2),
    _Step(q=_MIX_B, att=_MIX_A, prep=("wq", 3), load_wo=3, early=("wo_own", 1)),
    _Step(q=_own(REM, 3), att=_MIX_B, prep=("x", 3)),
    _Step(q=_tiles(REM, (3,), REM, ALL), att=_own(REM, 3), prep=("wo_own", 2)),
    _Step(att=_tiles(REM, (3,), REM, ALL), out=(REM, 0, 0, 2), early=("wo", 0)),
    _Step(out=(REM, 2, 0, 2)),
    _Step(q=_tiles(OWN, ALL, REM, (2,)), att=_tiles(OWN, ALL, REM, (1,)), prep=("wo_own", 3)),
    _Step(out=(REM, 0, 1, 4), early=("wo", 1)),
    _Step(q=_tiles(OWN, ALL, REM, (3,)), att=_tiles(OWN, ALL, REM, (2,))),
    _Step(att=_tiles(OWN, ALL, REM, (3,))),
    _Step(out=(REM, 0, 2, 4), early=("wo", 2)),
    _Step(out=(OWN, 0, 0, 4)),
    _Step(out=(OWN, 0, 1, 2)),
    _Step(out=(REM, 0, 3, 2), early=("wo", 3)),
    _Step(out=(REM, 2, 3, 2)),
    _Step(out=(OWN, 2, 1, 2)),
    _Step(out=(OWN, 0, 2, 4)),
)
WORDS = 4


def _aligned(i, n):
    return i if isinstance(i, int) else pl.multiple_of(i, n)


def _quadrant_sums(q11, q12, q21, q22):
    return (q11 + q22, q21 + q22, q11 + q12, q21 - q11, q12 - q22)


class _Strassen:
    ORDER = (0, 1, 2, 5, 3, 4, 6)

    def __init__(self, product, emit):
        self.product, self.emit, self.m = product, emit, {}

    def run(self, ts):
        for t in ts:
            m = self.m
            m[t] = self.product(t)
            done = lambda *need: t in need and all(k in m for k in need)
            if done(2, 4):
                self.emit(0, 1, m[2] + m[4])
            if done(1, 3):
                self.emit(1, 0, m[1] + m[3])
            if done(0, 3, 4, 6):
                self.emit(0, 0, m[0] + m[3] - m[4] + m[6])
            if done(0, 1, 2, 5):
                self.emit(1, 1, m[0] - m[1] + m[2] + m[5])


def _body(x_hbm, wq_hbm, k_hbm, v_hbm, wo_hbm, out,
          xf, wqf, wof, kvf, raw, sums, q_acc, qs, ctx, part_out, part_in, table,
          x_sem, wq_sem, wo_sem, kv_sem, blk_send, blk_recv, part_send, part_recv):
    me = lax.axis_index("i")
    row_peer = me ^ 1
    head_peer = 3 - me

    barrier = pltpu.get_barrier_semaphore()
    for peer in (row_peer, head_peer):
        pl.semaphore_signal(barrier, inc=1, device_id=(peer,), device_id_type=pl.DeviceIdType.MESH)

    def wq_load(q):
        rows = pl.ds(_aligned(256 * q, 256), 256)
        return pltpu.make_async_copy(wq_hbm.at[rows], wqf.at[q], wq_sem.at[q])

    def x_load(q):
        cols = pl.ds(_aligned(256 * q, 256), 256)
        return pltpu.make_async_copy(x_hbm.at[:, :, :, cols], xf.at[q], x_sem.at[q])

    def wo_load(n):
        return pltpu.make_async_copy(wo_hbm.at[:, pl.ds(_aligned(256 * n, 256), 256)], wof.at[n], wo_sem.at[n])

    def start_kv(group):
        first, r = 8 * jnp.where(group < 4, me, head_peer), group & 3
        for e, src in enumerate((k_hbm, v_hbm)):
            for h in range(8):
                pltpu.make_async_copy(src.at[:, r, :, first + h, :], kvf.at[group, e, h],
                                      kv_sem.at[group]).start()

    def block_copy(base, c, peer, part=()):
        sem = (base >> 1) + c
        return pltpu.make_async_remote_copy(
            raw.at[(base + c,) + part], raw.at[(base + 4 + c,) + part],
            blk_send.at[base >> 3], blk_recv.at[sem],
            device_id=(peer,), device_id_type=pl.DeviceIdType.MESH)

    def part_copy(r, n):
        return pltpu.make_async_remote_copy(
            part_out.at[4 * n + r], part_in.at[4 * n + r],
            part_send, part_recv.at[4 * n + r],
            device_id=(row_peer,), device_id_type=pl.DeviceIdType.MESH)

    def put_tile(blk, k, quad, store_raw=True):
        for h in range(2):
            rows = pl.ds(64 * h, 64)
            quads = [quad(a, b, h) for a in range(2) for b in range(2)]
            if store_raw:
                for i, q in enumerate(quads):
                    raw[blk, k, i, rows, :] = q.astype(BF16)
            for i, q in enumerate(_quadrant_sums(*quads)):
                sums[blk, k, i, rows, :] = q.astype(BF16)

    def prep_own_x(r, k):
        put_tile(X_BLK + r, k, lambda a, b, h: xf[k, 2 * a + h, r, :, pl.ds(128 * b, 128)])

    def prep_own_wq(j, k):
        put_tile(WQ_BLK + j, k, lambda a, b, h: wqf[
            k, pl.ds(128 * a + 64 * h, 64), pl.ds(256 * j + 128 * b, 128)] * Q_SCALE)

    def prep_own_wo(n):
        for k in range(4):
            put_tile(WO_BLK + n, k, lambda a, b, h: wof[
                n, pl.ds(256 * k + 128 * a + 64 * h, 64), pl.ds(128 * b, 128)])

    def prep_received(blk):
        for k in range(4):
            put_tile(blk, k, lambda a, b, h: raw[blk, k, 2 * a + b, pl.ds(64 * h, 64), :].astype(F32),
                     store_raw=False)

    def operand(blk, k, slot):
        return raw[blk, k, slot] if slot < 4 else sums[blk, k, slot - 4]

    def q_projection(sr, gj):
        xb, wb, tile = X_BLK + sr, WQ_BLK + gj, sr * 8 + gj

        def product(t):
            lhs = jnp.concatenate(
                [operand(xb, k, LHS_SLOT[t]) for k in range(4)], axis=1)
            rhs = jnp.concatenate([operand(wb, k, RHS_SLOT[t]) for k in range(4)], axis=0)
            return jnp.dot(lhs, rhs, preferred_element_type=F32)

        def emit(a, b, val):
            qs[2 * tile + b, 128 * a:128 * (a + 1), :] = val.astype(BF16)

        return _Strassen(product, emit)

    class Attention:
        def __init__(self, sr, gj):
            self.sr, self.gj = sr, gj
            self.p = {}

        def keys(self, which, e):
            block = kvf[(self.gj & 4) + (self.sr & 3), which, 2 * (self.gj & 3) + e]
            return block.reshape(256, 128).astype(BF16)

        def scores(self):
            for e in range(2):
                k = self.keys(0, e)
                q = qs[2 * (self.sr * 8 + self.gj) + e]
                s = lax.dot_general(q, k, (((1,), (1,)), ((), ())), preferred_element_type=F32)
                p = jnp.exp2(s - jnp.max(s, axis=-1, keepdims=True))
                self.p[e] = (p.astype(BF16), jnp.sum(p, axis=-1, keepdims=True))

        def values(self):
            o = []
            for e in range(2):
                p, l = self.p[e]
                v = self.keys(1, e)
                inv = pl.reciprocal(l, approx=True)
                inv = inv * (2.0 - l * inv)
                o.append(jnp.dot(p, v, preferred_element_type=F32) * inv)
            quads = (o[0][:128], o[1][:128], o[0][128:], o[1][128:])
            slots = quads + _quadrant_sums(*quads)
            for t in range(7):
                ctx[self.sr, t, self.gj] = slots[LHS_SLOT[t]].astype(BF16)

    def out_projection(s, rs, n, defer=None):
        def product(t):
            lhs = jnp.concatenate(
                [jnp.concatenate([ctx[4 * s + r, t, k] for k in range(8)], axis=1) for r in rs], axis=0)
            rhs = jnp.concatenate([operand(WO_BLK + 4 * g + n, k, RHS_SLOT[t])
                                   for g in range(2) for k in range(4)], axis=0)
            return jnp.dot(lhs, rhs, preferred_element_type=F32)

        def finish(r, a, b, val):
            val = val + part_in[4 * n + r, b, 128 * a:128 * (a + 1), :].astype(F32)
            for j in range(2):
                rows = pl.ds(_aligned(256 * (2 * a + j) + 64 * r, 64), 64)
                cols = pl.ds(_aligned(256 * n + 128 * b, 128), 128)
                out[0, rows, cols] = val[64 * j:64 * (j + 1)].astype(BF16)

        def emit(a, b, vals):
            for i, r in enumerate(rs):
                val = vals[128 * i:128 * (i + 1)]
                if s == REM:
                    part_out[4 * n + r, b, 128 * a:128 * (a + 1), :] = val.astype(BF16)
                elif defer and r in defer[0]:
                    defer[1].append(functools.partial(finish, r, a, b, val))
                else:
                    finish(r, a, b, val)

        return _Strassen(product, emit)

    for cp in (wq_load(0), x_load(0), wq_load(1)):
        cp.start()
    used = [st.kind for st in SCHEDULE]
    kinds = sorted(dict.fromkeys(used), key=used.count, reverse=True)
    for k, st in enumerate(SCHEDULE):
        for c, word in enumerate(st.words(kinds)):
            table[WORDS * k + c] = jnp.int32(word)

    def project(tiles):
        for tile in tiles:
            q_projection(*tile).run(_Strassen.ORDER)

    q_acc[...] = jnp.zeros(q_acc.shape, F32)
    pl.semaphore_wait(barrier, 2)

    def quarter(q, carry):
        wq_load(q).wait()
        pl.when(q < 3)(lambda: x_load(q + 1).start())
        prep_own_wq(0, q)
        block_copy(WQ_BLK, 0, head_peer, (q,)).start()
        for j in (1, 2, 3):
            prep_own_wq(j, q)

        @pl.when(q == 0)
        def _():
            block_copy(WQ_BLK, 1, head_peer, (0, pl.ds(0, 3))).start()

        @pl.when(q == 3)
        def _():
            block_copy(WQ_BLK, 1, head_peer, (0, pl.ds(3, 1))).start()
            block_copy(WQ_BLK, 1, head_peer, (pl.ds(1, 3),)).start()
            block_copy(WQ_BLK, 2, head_peer).start()
            block_copy(WQ_BLK, 3, head_peer).start()

        x_load(q).wait()
        pl.when(q < 2)(lambda: wq_load(q + 2).start())
        pl.when(q >= 2)(lambda: start_kv(q - 2))
        prep_own_x(0, q)
        prep_own_x(1, q)
        block_copy(X_BLK, 0, row_peer, (q,)).start()

        @pl.when(q == 0)
        def _():
            block_copy(X_BLK, 1, row_peer, (0, pl.ds(0, 3))).start()

        @pl.when(q == 3)
        def _():
            block_copy(X_BLK, 1, row_peer, (0, pl.ds(3, 1))).start()
            block_copy(X_BLK, 1, row_peer, (pl.ds(1, 3),)).start()

        for r in ALL:
            if r < 2:
                prep_own_x(r + 2, q)

            def product(t):
                rhs = jnp.concatenate([operand(WQ_BLK + j, q, RHS_SLOT[t]) for j in ALL], axis=1)
                return jnp.dot(operand(X_BLK + r, q, LHS_SLOT[t]), rhs, preferred_element_type=F32)

            def emit(a, b, val):
                for j in ALL:
                    total = q_acc[r, 2 * a + b, j] + val[:, 128 * j:128 * (j + 1)]
                    q_acc[r, 2 * a + b, j] = total
                    qs[2 * (8 * r + j) + b, 128 * a:128 * (a + 1), :] = total.astype(BF16)

            _Strassen(product, emit).run(_Strassen.ORDER)
        return carry

    lax.fori_loop(0, 4, quarter, None)
    for c in (2, 3):
        block_copy(X_BLK, c, row_peer).start()

    def run_step(row, kind):
        n_qp, n_at, op_shard, n_op, own_prep = kind
        unpack = lambda word, n: [((word >> (6 * a + 3)) & 7, (word >> (6 * a)) & 7) for a in range(n)]
        qp = unpack(row[0], n_qp)
        att = [Attention(*tile) for tile in unpack(row[1], n_at)]
        misc = row[2]
        base, c = (misc >> 8) & 24, (misc >> 8) & 3
        if own_prep:
            wo_load(c).wait()
        elif own_prep is not None:
            block_copy(base, c, row_peer).wait_recv()

        if op_shard >= 0:
            r0, n = (misc >> 4) & 2, (misc >> 6) & 3
            rs = (r0, r0 + 1) if n_op == 2 else ALL
            if op_shard == OWN:
                for r in rs:
                    part_copy(r, n).wait_recv()
            mm = out_projection(op_shard, rs, n)
            matmuls = [functools.partial(mm.run, ts) for ts in (_Strassen.ORDER[:4], _Strassen.ORDER[4:])]
        else:
            matmuls = [functools.partial(project, qp[a:a + 2]) for a in range(0, n_qp, 2)]

        if not att:
            for run in matmuls:
                run()
        elif not matmuls:
            for a in range(n_at + LOOKAHEAD):
                if a < n_at:
                    att[a].scores()
                if a >= LOOKAHEAD:
                    att[a - LOOKAHEAD].values()
        else:
            for a, run in enumerate(matmuls):
                att[2 * a].scores()
                att[2 * a + 1].scores()
                if a == 0 and own_prep:
                    prep_own_wo(c)
                elif a == 0 and own_prep is not None:
                    prep_received(base + 4 + c)
                run()
                att[2 * a].values()
                att[2 * a + 1].values()

        if own_prep:
            block_copy(WO_BLK, c, head_peer).start()
        if op_shard == REM:
            for r in rs:
                part_copy(r, n).start()

    def table_row(i):
        return tuple(table[WORDS * i + c] for c in range(WORDS))

    def step(i, row):
        next_row = table_row(jnp.minimum(i + 1, len(SCHEDULE) - 1))
        moves = row[3]

        @pl.when(moves != 0)
        def _():
            @pl.when((moves & 8) != 0)
            def _():
                group = kvf.at[moves & 7]
                pltpu.make_async_copy(group, group, kv_sem.at[moves & 7]).wait()

            pl.when((moves & (8 << 4)) != 0)(lambda: start_kv((moves >> 4) & 7))
            pl.when((moves & (4 << 8)) != 0)(lambda: wo_load((moves >> 8) & 3).start())
            base, c = (moves >> 12) & 24, (moves >> 12) & 3

            @pl.when((moves & (32 << 12)) != 0)
            def _():
                block_copy(base, c, row_peer).wait_recv()
                prep_received(base + 4 + c)

            @pl.when((moves & (64 << 12)) != 0)
            def _():
                wo_load(c).wait()
                prep_own_wo(c)
                block_copy(WO_BLK, c, head_peer).start()

        lax.switch(row[2] & 15, [functools.partial(run_step, row, kind) for kind in kinds])
        return next_row

    lax.fori_loop(0, len(SCHEDULE), step, table_row(0))

    for r in range(EARLY_PARTS):
        part_copy(r, 3).wait_recv()
    pending = []
    mm = out_projection(OWN, ALL, 3, defer=(range(EARLY_PARTS, 4), pending))
    mm.run(_Strassen.ORDER)
    for r in range(EARLY_PARTS, 4):
        part_copy(r, 3).wait_recv()
    for finish in pending:
        finish()

    for kind, base in enumerate((X_BLK, WQ_BLK, WO_BLK)):
        sent = raw.at[pl.ds(base, 4)]
        pltpu.make_async_copy(sent, sent, blk_send.at[kind]).wait()
    pltpu.make_async_copy(part_out, part_out, part_send).wait()


def pallas_dist_sparse_attn_strided_qseq_b1_sq1024_skv1024_hq8_dh128_kernel(
    x: jax.Array,
    Wq: jax.Array,
    K_ext: jax.Array,
    V_ext: jax.Array,
    Wo: jax.Array,
):
    dma = pltpu.SemaphoreType.DMA
    return pl.pallas_call(
        _body,
        out_shape=pltpu.VMEM((1, 1024, 1024), BF16),
        in_specs=[pl.BlockSpec(memory_space=pl.ANY)] * 5,
        out_specs=pl.BlockSpec(memory_space=pltpu.VMEM),
        scratch_shapes=[
            pltpu.VMEM((4, 4, 4, 64, 256), F32),
            pltpu.VMEM((4, 256, 1024), F32),
            pltpu.VMEM((4, 1024, 256), F32),
            pltpu.VMEM((8, 2, 8, 4, 64, 128), F32),
            pltpu.VMEM((24, 4, 4, 128, 128), BF16),
            pltpu.VMEM((24, 4, 5, 128, 128), BF16),
            pltpu.VMEM((4, 4, 4, 128, 128), F32),
            pltpu.VMEM((128, 256, 128), BF16),
            pltpu.VMEM((8, 7, 8, 128, 128), BF16),
            pltpu.VMEM((16, 2, 256, 128), BF16),
            pltpu.VMEM((16, 2, 256, 128), BF16),
            pltpu.SMEM((WORDS * len(SCHEDULE),), jnp.int32),
            dma((4,)), dma((4,)), dma((4,)), dma((8,)),
            dma((3,)), dma((12,)), dma, dma((16,)),
        ],
        compiler_params=pltpu.CompilerParams(collective_id=0, vmem_limit_bytes=100 * 1024 * 1024),
    )(
        x.reshape(4, 4, 64, 1024),
        Wq,
        K_ext.reshape(4, 4, 64, 32, 128),
        V_ext.reshape(4, 4, 64, 32, 128),
        Wo,
    )
```
